```python
import numpy as np

kernel_name = "dist_argmax_global_i_m4096_n1024"

def setup_inputs():
    return {"x": np.random.randn(16384, 1024).astype(np.float32)}

def reference(x: np.ndarray) -> np.ndarray:
    idx = np.argmax(x, axis=0).astype(np.float32)
    val = np.max(x, axis=0)
    return np.stack([val, idx], axis=0)
```

```python
import functools

import jax
import jax.numpy as jnp
from jax import lax
from jax.experimental import pallas as pl
from jax.experimental.pallas import tpu as pltpu

N_DEV = 4
M = 4096
N = 1024
H = N // 2
SUB = 8

LOCAL_CHUNKS = (2048, 768, 512, 256)
TAIL = 128
RIGHT_SPLIT = (24, 8)
PUSHED = 192
CONSUME_PUSHED_AFTER = 1
UNROLL = 8
STATIC_TILES = 16

TAIL_START = sum(LOCAL_CHUNKS)
PUSH_START = TAIL_START + TAIL
assert PUSH_START + 2 * PUSHED == M


def _pieces():
    out, row = [], 0
    for n in LOCAL_CHUNKS:
        out.append((row, n, (0, 1)))
        row += n
    out.append((TAIL_START, TAIL, (0,)))
    row = TAIL_START
    for n in (TAIL - sum(RIGHT_SPLIT),) + RIGHT_SPLIT:
        out.append((row, n, (1,)))
        row += n
    return tuple(out)


PIECES = _pieces()
LAST_PIECE = tuple(
    max(i for i, (_, _, hs) in enumerate(PIECES) if hs == (h,)) for h in (0, 1)
)


def _update(v, cur, idx, row):
    cand = jnp.where(v <= cur, idx, row)
    idx = jnp.where(cur == cur, cand, idx)
    return jnp.maximum(cur, v), idx


def _candidate(v, best, i):
    return jnp.where(v != v, i, jnp.where(v == best, i, jnp.inf))


def _merge(a, b):
    (av, ai), (bv, bi) = a, b
    best = jnp.maximum(av, bv)
    return best, jnp.minimum(_candidate(av, best, ai), _candidate(bv, best, bi))


def _reduce_rows(cur, idx, other=None):
    best = jnp.max(cur, axis=0, keepdims=True)
    if other is not None:
        best = jnp.maximum(best, other[0])
    arg = jnp.min(_candidate(cur, best, idx), axis=0, keepdims=True)
    if other is not None:
        arg = jnp.minimum(arg, _candidate(other[0], best, other[1]))
    return best, arg


def _scan_rows(buf, first, nrows, halves, state, row):
    def step(t, carry):
        *st, row = carry
        r = pl.multiple_of(first + t * SUB, SUB)
        for j, h in enumerate(halves):
            v = buf[pl.ds(r, SUB), pl.ds(h * H, H)]
            st[2 * j], st[2 * j + 1] = _update(v, st[2 * j], st[2 * j + 1], row)
        return (*st, row + float(SUB))

    carry = tuple(state[2 * h + i] for h in halves for i in range(2)) + (row,)
    ntiles = nrows // SUB
    if ntiles <= STATIC_TILES:
        for t in range(ntiles):
            carry = step(t, carry)
    else:
        carry = lax.fori_loop(0, ntiles, step, carry, unroll=UNROLL)
    state = list(state)
    for j, h in enumerate(halves):
        state[2 * h], state[2 * h + 1] = carry[2 * j], carry[2 * j + 1]
    return state


def _stream_and_send(x_hbm, xbuf, pushed, part, recv, recv_sem, push_sem,
                     load_sems, send_sem):
    me = lax.axis_index("i")
    right = lax.rem(me + 1, N_DEV)
    left = lax.rem(me + N_DEV - 1, N_DEV)

    loads = []
    for i, (first, n, halves) in enumerate(PIECES):
        cols = pl.ds(0, N) if len(halves) == 2 else pl.ds(halves[0] * H, H)
        loads.append(pltpu.make_async_copy(
            x_hbm.at[pl.ds(first, n), cols], xbuf.at[pl.ds(first, n), cols],
            load_sems.at[i]))
    pushes = [
        pltpu.make_async_remote_copy(
            x_hbm.at[pl.ds(PUSH_START + j * PUSHED, PUSHED)],
            pushed.at[pl.ds(j * PUSHED, PUSHED)],
            send_sem, push_sem,
            device_id=(dst,), device_id_type=pl.DeviceIdType.MESH)
        for j, dst in enumerate((right, left))
    ]

    for cp in loads:
        cp.start()
    barrier = pltpu.get_barrier_semaphore()
    for nbr in (left, right):
        pl.semaphore_signal(barrier, inc=1, device_id=(nbr,),
                            device_id_type=pl.DeviceIdType.MESH)
    pl.semaphore_wait(barrier, 2)
    for cp in pushes:
        cp.start()

    sublane = lax.broadcasted_iota(jnp.int32, (SUB, H), 0).astype(jnp.float32)
    neg_inf = jnp.full((SUB, H), -jnp.inf, jnp.float32)
    base = (me * M).astype(jnp.float32) + sublane
    state = [neg_inf, base, neg_inf, base]
    pushed_part = None
    sends = []
    for i, (first, n, halves) in enumerate(PIECES):
        loads[i].wait()
        state = _scan_rows(xbuf, first, n, halves, state, base + float(first))
        if i == CONSUME_PUSHED_AFTER:
            pltpu.make_async_copy(pushed, pushed, push_sem).wait()
            blocks = []
            for j, src in enumerate((left, right)):
                row = (src * M + PUSH_START + j * PUSHED).astype(jnp.float32) + sublane
                blocks.append(_scan_rows(pushed, j * PUSHED, PUSHED, (0, 1),
                                         [neg_inf, row, neg_inf, row], row))
            pushed_part = [
                _reduce_rows(*_merge(blocks[0][2 * h:2 * h + 2],
                                     blocks[1][2 * h:2 * h + 2]))
                for h in (0, 1)
            ]
        for h in (0, 1):
            if i == LAST_PIECE[h]:
                best, arg = _reduce_rows(state[2 * h], state[2 * h + 1],
                                         pushed_part[h])
                cols = pl.ds(h * H, H)
                part[0:1, cols] = best
                part[1:2, cols] = arg
                for k in (2, 1, 3):
                    cp = pltpu.make_async_remote_copy(
                        part.at[:, cols], recv.at[k - 1, :, cols],
                        send_sem, recv_sem,
                        device_id=(lax.rem(me + k, N_DEV),),
                        device_id_type=pl.DeviceIdType.MESH)
                    cp.start()
                    sends.append(cp)
    for cp in pushes + sends:
        cp.wait_send()


def _kernel(x_hbm, out_ref, xbuf, pushed, part, recv, recv_sem, push_sem):
    pl.run_scoped(
        functools.partial(_stream_and_send, x_hbm, xbuf, pushed, part, recv,
                          recv_sem, push_sem),
        pltpu.SemaphoreType.DMA((len(PIECES),)),
        pltpu.SemaphoreType.DMA,
    )
    pltpu.make_async_copy(recv, recv, recv_sem).wait()
    vals = [part[0:1, :]] + [recv[k, 0:1, :] for k in range(N_DEV - 1)]
    args = [part[1:2, :]] + [recv[k, 1:2, :] for k in range(N_DEV - 1)]
    best = functools.reduce(jnp.maximum, vals)
    arg = functools.reduce(
        jnp.minimum, [_candidate(v, best, i) for v, i in zip(vals, args)])
    out_ref[0:1, :] = best
    out_ref[1:2, :] = arg


def pallas_dist_argmax_global_i_m4096_n1024_kernel(x: jax.Array):
    assert x.shape == (M, N) and x.dtype == jnp.float32, (x.shape, x.dtype)
    return pl.pallas_call(
        _kernel,
        out_shape=jax.ShapeDtypeStruct((2, N), jnp.float32),
        in_specs=[pl.BlockSpec(memory_space=pl.ANY)],
        out_specs=pl.BlockSpec(memory_space=pltpu.VMEM),
        scratch_shapes=[
            pltpu.VMEM((PUSH_START, N), jnp.float32),
            pltpu.VMEM((2 * PUSHED, N), jnp.float32),
            pltpu.VMEM((2, N), jnp.float32),
            pltpu.VMEM((N_DEV - 1, 2, N), jnp.float32),
            pltpu.SemaphoreType.DMA,
            pltpu.SemaphoreType.DMA,
        ],
        compiler_params=pltpu.CompilerParams(
            collective_id=0, vmem_limit_bytes=32 * 2**20),
    )(x)
```

```python
import functools

import jax
import jax.numpy as jnp
from jax import lax
from jax.experimental import pallas as pl
from jax.experimental.pallas import tpu as pltpu

N_DEV = 4
M = 4096
N = 1024
H = N // 2
SUB = 8

LOCAL_CHUNKS = (2048, 768, 496, 256)
TAIL = 128
RIGHT_SPLIT = (24, 8)
PUSHED = 200
CONSUME_PUSHED_AFTER = 2
UNROLL = 8
STATIC_TILES = 16

TAIL_START = sum(LOCAL_CHUNKS)
PUSH_START = TAIL_START + TAIL
assert PUSH_START + 2 * PUSHED == M


def _pieces():
    out, row = [], 0
    for n in LOCAL_CHUNKS:
        out.append((row, n, (0, 1)))
        row += n
    out.append((TAIL_START, TAIL, (0,)))
    row = TAIL_START
    for n in (TAIL - sum(RIGHT_SPLIT),) + RIGHT_SPLIT:
        out.append((row, n, (1,)))
        row += n
    return tuple(out)


PIECES = _pieces()
LAST_PIECE = tuple(
    max(i for i, (_, _, hs) in enumerate(PIECES) if hs == (h,)) for h in (0, 1)
)


def _update(v, cur, idx, row):
    cand = jnp.where(v <= cur, idx, row)
    idx = jnp.where(cur == cur, cand, idx)
    return jnp.maximum(cur, v), idx


def _candidate(v, best, i):
    return jnp.where(v != v, i, jnp.where(v == best, i, jnp.inf))


def _merge(a, b):
    (av, ai), (bv, bi) = a, b
    best = jnp.maximum(av, bv)
    return best, jnp.minimum(_candidate(av, best, ai), _candidate(bv, best, bi))


def _reduce_rows(cur, idx, other=None):
    best = jnp.max(cur, axis=0, keepdims=True)
    if other is not None:
        best = jnp.maximum(best, other[0])
    arg = jnp.min(_candidate(cur, best, idx), axis=0, keepdims=True)
    if other is not None:
        arg = jnp.minimum(arg, _candidate(other[0], best, other[1]))
    return best, arg


def _scan_rows(buf, first, nrows, halves, state, row):
    def step(t, carry):
        *st, row = carry
        r = pl.multiple_of(first + t * SUB, SUB)
        for j, h in enumerate(halves):
            v = buf[pl.ds(r, SUB), pl.ds(h * H, H)]
            st[2 * j], st[2 * j + 1] = _update(v, st[2 * j], st[2 * j + 1], row)
        return (*st, row + float(SUB))

    carry = tuple(state[2 * h + i] for h in halves for i in range(2)) + (row,)
    ntiles = nrows // SUB
    if ntiles <= STATIC_TILES:
        for t in range(ntiles):
            carry = step(t, carry)
    else:
        carry = lax.fori_loop(0, ntiles, step, carry, unroll=UNROLL)
    state = list(state)
    for j, h in enumerate(halves):
        state[2 * h], state[2 * h + 1] = carry[2 * j], carry[2 * j + 1]
    return state


def _stream_and_send(x_hbm, xbuf, pushed, part, recv, recv_sem, push_sem,
                     load_sems, send_sems):
    me = lax.axis_index("i")
    right = lax.rem(me + 1, N_DEV)
    left = lax.rem(me + N_DEV - 1, N_DEV)

    loads = []
    for i, (first, n, halves) in enumerate(PIECES):
        cols = pl.ds(0, N) if len(halves) == 2 else pl.ds(halves[0] * H, H)
        loads.append(pltpu.make_async_copy(
            x_hbm.at[pl.ds(first, n), cols], xbuf.at[pl.ds(first, n), cols],
            load_sems.at[i]))
    pushes = [
        pltpu.make_async_remote_copy(
            x_hbm.at[pl.ds(PUSH_START + j * PUSHED, PUSHED)],
            pushed.at[pl.ds(j * PUSHED, PUSHED)],
            send_sems.at[j], push_sem,
            device_id=(dst,), device_id_type=pl.DeviceIdType.MESH)
        for j, dst in enumerate((right, left))
    ]

    for cp in loads:
        cp.start()
    barrier = pltpu.get_barrier_semaphore()
    for k in range(1, N_DEV):
        pl.semaphore_signal(barrier, inc=1, device_id=(lax.rem(me + k, N_DEV),),
                            device_id_type=pl.DeviceIdType.MESH)
    pl.semaphore_wait(barrier, N_DEV - 1)
    for cp in pushes:
        cp.start()

    sublane = lax.broadcasted_iota(jnp.int32, (SUB, H), 0).astype(jnp.float32)
    neg_inf = jnp.full((SUB, H), -jnp.inf, jnp.float32)
    base = (me * M).astype(jnp.float32) + sublane
    state = [neg_inf, base, neg_inf, base]
    pushed_part = None
    sends = []
    for i, (first, n, halves) in enumerate(PIECES):
        loads[i].wait()
        state = _scan_rows(xbuf, first, n, halves, state, base + float(first))
        if i == CONSUME_PUSHED_AFTER:
            pltpu.make_async_copy(pushed, pushed, push_sem).wait()
            blocks = []
            for j, src in enumerate((left, right)):
                row = (src * M + PUSH_START + j * PUSHED).astype(jnp.float32) + sublane
                blocks.append(_scan_rows(pushed, j * PUSHED, PUSHED, (0, 1),
                                         [neg_inf, row, neg_inf, row], row))
            pushed_part = [
                _reduce_rows(*_merge(blocks[0][2 * h:2 * h + 2],
                                     blocks[1][2 * h:2 * h + 2]))
                for h in (0, 1)
            ]
        for h in (0, 1):
            if i == LAST_PIECE[h]:
                best, arg = _reduce_rows(state[2 * h], state[2 * h + 1],
                                         pushed_part[h])
                cols = pl.ds(h * H, H)
                part[0:1, cols] = best
                part[1:2, cols] = arg
                for k in (2, 1, 3):
                    cp = pltpu.make_async_remote_copy(
                        part.at[:, cols], recv.at[k - 1, :, cols],
                        send_sems.at[len(pushes) + len(sends)], recv_sem,
                        device_id=(lax.rem(me + k, N_DEV),),
                        device_id_type=pl.DeviceIdType.MESH)
                    cp.start()
                    sends.append(cp)
    for cp in pushes + sends:
        cp.wait_send()


def _kernel(x_hbm, out_ref, xbuf, pushed, part, recv, recv_sem, push_sem):
    pl.run_scoped(
        functools.partial(_stream_and_send, x_hbm, xbuf, pushed, part, recv,
                          recv_sem, push_sem),
        pltpu.SemaphoreType.DMA((len(PIECES),)),
        pltpu.SemaphoreType.DMA((2 + 2 * (N_DEV - 1),)),
    )
    pltpu.make_async_copy(recv, recv, recv_sem).wait()
    vals = [part[0:1, :]] + [recv[k, 0:1, :] for k in range(N_DEV - 1)]
    args = [part[1:2, :]] + [recv[k, 1:2, :] for k in range(N_DEV - 1)]
    best = functools.reduce(jnp.maximum, vals)
    arg = functools.reduce(
        jnp.minimum, [_candidate(v, best, i) for v, i in zip(vals, args)])
    out_ref[0:1, :] = best
    out_ref[1:2, :] = arg


def pallas_dist_argmax_global_i_m4096_n1024_kernel(x: jax.Array):
    assert x.shape == (M, N) and x.dtype == jnp.float32, (x.shape, x.dtype)
    return pl.pallas_call(
        _kernel,
        out_shape=jax.ShapeDtypeStruct((2, N), jnp.float32),
        in_specs=[pl.BlockSpec(memory_space=pl.ANY)],
        out_specs=pl.BlockSpec(memory_space=pltpu.VMEM),
        scratch_shapes=[
            pltpu.VMEM((PUSH_START, N), jnp.float32),
            pltpu.VMEM((2 * PUSHED, N), jnp.float32),
            pltpu.VMEM((2, N), jnp.float32),
            pltpu.VMEM((N_DEV - 1, 2, N), jnp.float32),
            pltpu.SemaphoreType.DMA,
            pltpu.SemaphoreType.DMA,
        ],
        compiler_params=pltpu.CompilerParams(
            collective_id=0, vmem_limit_bytes=32 * 2**20),
    )(x)
```

```python
import functools

import jax
import jax.numpy as jnp
from jax import lax
from jax.experimental import pallas as pl
from jax.experimental.pallas import tpu as pltpu

N_DEV = 4
M = 4096
N = 1024
SUB = 8

LOCAL_CHUNKS = (2048, 768, 496, 256)
TAIL = 128
GROUPS = ((0, 512, ()), (512, 256, ()), (768, 128, ()), (896, 128, (8,)))
PUSHED = 200
CONSUME_PUSHED_AFTER = 2
UNROLL = 8
STATIC_TILES = 16

TAIL_START = sum(LOCAL_CHUNKS)
PUSH_START = TAIL_START + TAIL
ALL_GROUPS = tuple(range(len(GROUPS)))
assert PUSH_START + 2 * PUSHED == M
assert sum(w for _, w, _ in GROUPS) == N


def _pieces():
    out, row = [], 0
    for n in LOCAL_CHUNKS:
        out.append((row, n, ALL_GROUPS))
        row += n
    for g, (_, _, small) in enumerate(GROUPS):
        row = TAIL_START
        for n in (TAIL - sum(small),) + small:
            out.append((row, n, (g,)))
            row += n
    return tuple(out)


PIECES = _pieces()
LAST_PIECE = tuple(
    max(i for i, (_, _, gs) in enumerate(PIECES) if gs == (g,)) for g in ALL_GROUPS
)


def _cols(groups):
    return pl.ds(GROUPS[groups[0]][0], sum(GROUPS[g][1] for g in groups))


def _row_ids(first_row, g):
    iota = lax.broadcasted_iota(jnp.int32, (SUB, GROUPS[g][1]), 0)
    return first_row + iota.astype(jnp.float32)


def _empty_state(first_row):
    return [(jnp.full((SUB, w), -jnp.inf, jnp.float32), _row_ids(first_row, g))
            for g, (_, w, _) in enumerate(GROUPS)]


def _update(v, cur, idx, row):
    cand = jnp.where(v <= cur, idx, row)
    idx = jnp.where(cur == cur, cand, idx)
    return jnp.maximum(cur, v), idx


def _candidate(v, best, i):
    return jnp.where(v != v, i, jnp.where(v == best, i, jnp.inf))


def _merge(a, b):
    (av, ai), (bv, bi) = a, b
    best = jnp.maximum(av, bv)
    return best, jnp.minimum(_candidate(av, best, ai), _candidate(bv, best, bi))


def _reduce_rows(cur, idx, other=None):
    best = jnp.max(cur, axis=0, keepdims=True)
    if other is not None:
        best = jnp.maximum(best, other[0])
    arg = jnp.min(_candidate(cur, best, idx), axis=0, keepdims=True)
    if other is not None:
        arg = jnp.minimum(arg, _candidate(other[0], best, other[1]))
    return best, arg


def _scan_rows(buf, first, nrows, groups, state, first_row):
    def step(t, carry):
        r = pl.multiple_of(first + t * SUB, SUB)
        out = []
        for g, ((cur, idx), row) in zip(groups, carry):
            v = buf[pl.ds(r, SUB), _cols((g,))]
            out.append((_update(v, cur, idx, row), row + float(SUB)))
        return tuple(out)

    carry = tuple((state[g], _row_ids(first_row, g)) for g in groups)
    ntiles = nrows // SUB
    if ntiles <= STATIC_TILES:
        for t in range(ntiles):
            carry = step(t, carry)
    else:
        carry = lax.fori_loop(0, ntiles, step, carry, unroll=UNROLL)
    state = list(state)
    for g, (st, _) in zip(groups, carry):
        state[g] = st
    return state


def _stream_and_send(x_hbm, xbuf, pushed, part, recv, recv_sem, push_sem,
                     load_sems, send_sems):
    me = lax.axis_index("i")
    right = lax.rem(me + 1, N_DEV)
    left = lax.rem(me + N_DEV - 1, N_DEV)

    loads = [
        pltpu.make_async_copy(
            x_hbm.at[pl.ds(first, n), _cols(groups)],
            xbuf.at[pl.ds(first, n), _cols(groups)],
            load_sems.at[i])
        for i, (first, n, groups) in enumerate(PIECES)
    ]
    pushes = [
        pltpu.make_async_remote_copy(
            x_hbm.at[pl.ds(PUSH_START + j * PUSHED, PUSHED)],
            pushed.at[pl.ds(j * PUSHED, PUSHED)],
            send_sems.at[j], push_sem,
            device_id=(dst,), device_id_type=pl.DeviceIdType.MESH)
        for j, dst in enumerate((right, left))
    ]

    for cp in loads:
        cp.start()
    barrier = pltpu.get_barrier_semaphore()
    for k in range(1, N_DEV):
        pl.semaphore_signal(barrier, inc=1, device_id=(lax.rem(me + k, N_DEV),),
                            device_id_type=pl.DeviceIdType.MESH)
    pl.semaphore_wait(barrier, N_DEV - 1)
    for cp in pushes:
        cp.start()

    base = (me * M).astype(jnp.float32)
    state = _empty_state(base)
    pushed_part = None
    sends = []
    for i, (first, n, groups) in enumerate(PIECES):
        loads[i].wait()
        state = _scan_rows(xbuf, first, n, groups, state, base + float(first))
        if i == CONSUME_PUSHED_AFTER:
            pltpu.make_async_copy(pushed, pushed, push_sem).wait()
            blocks = []
            for j, src in enumerate((left, right)):
                row = (src * M + PUSH_START + j * PUSHED).astype(jnp.float32)
                blocks.append(_scan_rows(pushed, j * PUSHED, PUSHED, ALL_GROUPS,
                                         _empty_state(row), row))
            pushed_part = [_reduce_rows(*_merge(a, b)) for a, b in zip(*blocks)]
        for g in ALL_GROUPS:
            if i == LAST_PIECE[g]:
                best, arg = _reduce_rows(*state[g], pushed_part[g])
                cols = _cols((g,))
                part[0:1, cols] = best
                part[1:2, cols] = arg
                for k in (2, 1, 3):
                    cp = pltpu.make_async_remote_copy(
                        part.at[:, cols], recv.at[k - 1, :, cols],
                        send_sems.at[len(pushes) + len(sends)], recv_sem,
                        device_id=(lax.rem(me + k, N_DEV),),
                        device_id_type=pl.DeviceIdType.MESH)
                    cp.start()
                    sends.append(cp)
    for cp in pushes + sends:
        cp.wait_send()


def _kernel(x_hbm, out_ref, xbuf, pushed, part, recv, recv_sem, push_sem):
    pl.run_scoped(
        functools.partial(_stream_and_send, x_hbm, xbuf, pushed, part, recv,
                          recv_sem, push_sem),
        pltpu.SemaphoreType.DMA((len(PIECES),)),
        pltpu.SemaphoreType.DMA((2 + len(GROUPS) * (N_DEV - 1),)),
    )
    pltpu.make_async_copy(recv, recv, recv_sem).wait()
    vals = [part[0:1, :]] + [recv[k, 0:1, :] for k in range(N_DEV - 1)]
    args = [part[1:2, :]] + [recv[k, 1:2, :] for k in range(N_DEV - 1)]
    best = functools.reduce(jnp.maximum, vals)
    arg = functools.reduce(
        jnp.minimum, [_candidate(v, best, i) for v, i in zip(vals, args)])
    out_ref[0:1, :] = best
    out_ref[1:2, :] = arg


def pallas_dist_argmax_global_i_m4096_n1024_kernel(x: jax.Array):
    assert x.shape == (M, N) and x.dtype == jnp.float32, (x.shape, x.dtype)
    return pl.pallas_call(
        _kernel,
        out_shape=jax.ShapeDtypeStruct((2, N), jnp.float32),
        in_specs=[pl.BlockSpec(memory_space=pl.ANY)],
        out_specs=pl.BlockSpec(memory_space=pltpu.VMEM),
        scratch_shapes=[
            pltpu.VMEM((PUSH_START, N), jnp.float32),
            pltpu.VMEM((2 * PUSHED, N), jnp.float32),
            pltpu.VMEM((2, N), jnp.float32),
            pltpu.VMEM((N_DEV - 1, 2, N), jnp.float32),
            pltpu.SemaphoreType.DMA,
            pltpu.SemaphoreType.DMA,
        ],
        compiler_params=pltpu.CompilerParams(
            collective_id=0, vmem_limit_bytes=32 * 2**20),
    )(x)
```
